```python
import numpy as np

kernel_name = "dist_sparse_attn_blocksparse_qseq_b2_sq256_skv256_hq4_dh64"

def setup_inputs():
    x = np.random.randn(2, 1024, 512).astype(np.float32)
    Wq = np.random.randn(512, 1024).astype(np.float32) * 0.02
    K_ext = np.random.randn(2, 256, 16, 64).astype(np.float32)
    V_ext = np.random.randn(2, 256, 16, 64).astype(np.float32)
    Wo = np.random.randn(1024, 512).astype(np.float32) * 0.02
    return {"x": x, "Wq": Wq, "K_ext": K_ext, "V_ext": V_ext, "Wo": Wo}

def reference(x, Wq, K_ext, V_ext, Wo):
    B, Sq, Skv, Hq, Dh = 2, 1024, 256, 16, 64
    Q = (x @ Wq).reshape(B, Sq, Hq, Dh)
    qb = (np.arange(Sq) // 64)[:, None]
    kb = (np.arange(Skv) // 64)[None, :]
    mask = (qb == kb) | (kb == 0) | ((qb + kb) % 3 == 0)
    scores = np.einsum('bihd,bjhd->bhij', Q, K_ext).astype(np.float32) * 0.125
    scores = np.where(mask[None, None, :, :], scores, -1e9)
    scores_max = scores.max(axis=-1, keepdims=True)
    w = np.exp(scores - scores_max)
    row_keep = mask.any(axis=1)
    w_sum = np.where(row_keep[None, None, :, None], w.sum(axis=-1, keepdims=True), 1.0)
    w = w / w_sum
    w = np.where(row_keep[None, None, :, None], w, 0.0)
    ctx = np.einsum('bhij,bjhd->bihd', w, V_ext).reshape(B, Sq, Hq * Dh)
    return ctx @ Wo
```

```python
import jax
import jax.numpy as jnp
import numpy as np
from jax import lax
from jax.experimental import pallas as pl
from jax.experimental.pallas import tpu as pltpu

N_DEV = 4
B, SQ, D, SKV, DH, BLK = 2, 256, 512, 256, 64, 64
ROWS = B * SQ
PAIR = 2 * DH
LOG2E = 1.4426950408889634
SCORE_SCALE = 0.125 * LOG2E
MASKED = -1e9 * LOG2E
MESH = pl.DeviceIdType.MESH
BF16, F32, U32, I32 = jnp.bfloat16, jnp.float32, jnp.uint32, jnp.int32


def _allowed(qb, kb):
  return (qb == kb) | (kb == 0) | ((qb + kb) % 3 == 0)


for _qb in (4 * _d + _j for _d in range(N_DEV) for _j in (0, 3)):
  assert set(np.flatnonzero(_allowed(_qb, np.arange(4)))) == {0, 3 - _qb % 3}

WORDS = 32
HEADER, BODY = 6, 8
PLACES = 5
PACKET_ROWS = BODY + 8 * (3 * WORDS // 4)
SPREAD = (((11, 0, 4),), ((11, 4, 4),), ((11, 8, 3), (14, 15, 1)))
WQ_CHUNKS = (2, 2, 4, 8, 16)
WO_TAIL = (0, 4, 6, 7, 8)


def _u32(c):
  return jnp.uint32(c & 0xFFFFFFFF)


def _shift(v, n):
  if n == 0:
    return v
  return v << _u32(n) if n > 0 else v >> _u32(-n)


def _bits(pos, width):
  return (((1 << width) - 1) << pos) * 0x00010001


def _to_words(v):
  return pltpu.bitcast(v.astype(BF16), U32)


def _from_words(v):
  return pltpu.bitcast(v, BF16)


def _lowest_exponent(values, margin):
  top = jnp.max(jnp.abs(values), axis=0, keepdims=True) * margin
  exponent = (pltpu.bitcast(top, I32) >> 23) & 0xFF
  return jnp.maximum(exponent - 31, 0).astype(U32)


def _offset(lowest):
  return (lowest << _u32(7)) | (lowest << _u32(23))


def _write_carriers(packet, rel, carriers):
  for c in carriers:
    g, i = divmod(c, 3)
    v = rel[4 * g + 1 + i] & _u32(~_bits(11, 4))
    for carrier_bit, bit, width in SPREAD[i]:
      v = v | _shift(rel[4 * g] & _u32(_bits(bit, width)), carrier_bit - bit)
    packet[pl.ds(BODY + 8 * c, 8), :] = v


def _one_hot(i):
  one = _u32(0x80000000) >> (i & _u32(31))
  zero = jnp.zeros_like(one)
  return jnp.where(i < _u32(32), one, zero), jnp.where((i >> _u32(5)) == _u32(1), one, zero)


def _sublane():
  return lax.broadcasted_iota(I32, (8, 128), 0).astype(U32)


def _list_clear_bits(rel):
  planes = []
  for h in range(2):
    plane = None
    for i in range(16):
      t = _shift(~rel[16 * h + i] & _u32(_bits(11, 1)), i - 11)
      plane = t if plane is None else plane | t
    planes.append(plane)
  a, b = planes
  places = []
  for _ in range(PLACES):
    i = jnp.where(a != 0, lax.clz(a), _u32(32) + lax.clz(b))
    place = (i << _u32(3)) | _sublane()
    first = jnp.min(place.astype(I32), axis=0, keepdims=True).astype(U32)
    hot_a, hot_b = _one_hot(jnp.where(place == first, i, _u32(64)))
    a, b = a & ~hot_a, b & ~hot_b
    places.append(first)
  return places, a | b


def _write_header(packet, places, note):
  for row, (p, q, r) in enumerate((places[:3], (*places[3:], note))):
    packet[pl.ds(HEADER + row, 1), :] = p | (q << _u32(10)) | (r << _u32(20))


def _read_header(packet):
  rows = [packet[pl.ds(HEADER + row, 1), :] for row in range(2)]
  a = b = None
  for k in range(PLACES):
    place = (rows[k // 3] >> _u32(10 * (k % 3))) & _u32(0x3FF)
    hot_a, hot_b = _one_hot(jnp.where((place & _u32(7)) == _sublane(), place >> _u32(3), _u32(64)))
    a, b = (hot_a, hot_b) if a is None else (a | hot_a, b | hot_b)
  note = rows[1] >> _u32(20)
  return (a, b), _offset(note & _u32(0xFF)) + _u32(_bits(11, 1)), note >> _u32(8)


def _read_words(packet, header, words):
  planes, offset, _ = header
  carrier = lambda c: packet[pl.ds(BODY + 8 * c, 8), :]
  out = []
  for w in words:
    g, i = divmod(w, 4)
    if i:
      v = carrier(3 * g + i - 1) & _u32(~_bits(11, 4))
    else:
      v = None
      for c in range(3):
        for carrier_bit, bit, width in SPREAD[c]:
          part = _shift(carrier(3 * g + c) & _u32(_bits(carrier_bit, width)), bit - carrier_bit)
          v = part if v is None else v | part
    clear = _shift(planes[w // 16], 11 - w % 16) & _u32(_bits(11, 1))
    out.append(v - clear + offset)
  return _from_words(jnp.concatenate(out, axis=0))


def _kernel(x_hbm, wq_hbm, kt_hbm, vt_hbm, wo_hbm, out_ref,
            x_f32, wq_f32, wo_f32, kt_f32, vt_f32, q_buf, ctx_buf, acc_buf,
            wq_pkt, wo_pkt, wq_raw, wo_raw,
            load_sem, wq_send, wq_recv, wo_send, wo_recv, raw_send, raw_recv, ready_sem):
  n_chunks = len(WQ_CHUNKS)
  word_at = [sum(WQ_CHUNKS[:c]) for c in range(n_chunks + 1)]
  carrier_at = [3 * (w // 4) + max(w % 4 - 1, 0) for w in word_at]

  loads = {}

  def load(name, src, dst):
    sem = load_sem.at[sum(len(copies) for copies in loads.values())]
    loads.setdefault(name, []).append(pltpu.make_async_copy(src, dst, sem))
    loads[name][-1].start()

  def loaded(name):
    for copy in loads[name]:
      copy.wait()

  my = lax.axis_index("i")
  pair_order = [(my == 1).astype(I32) ^ i for i in range(2)]
  for i, e in enumerate(pair_order):
    cols = pl.ds(pl.multiple_of(PAIR * e, PAIR), PAIR)
    for c in range(n_chunks):
      rows = pl.ds(16 * word_at[c], 16 * WQ_CHUNKS[c])
      load(("wq", i, c), wq_hbm.at[rows, cols], wq_f32.at[i, rows])

  right, opposite, left = (my + 1) & 3, (my + 2) & 3, (my + 3) & 3
  neighbour = (right, left)
  odd = (my & 1) == 1

  barrier = pltpu.get_barrier_semaphore()

  @pl.when(my != 2)
  def _():
    for n in neighbour:
      pl.semaphore_signal(barrier, 1, device_id=(n,), device_id_type=MESH)

  pairs = (
      (2 * my, 2 * my + 1),
      (2 * left, 2 * right + 1),
      (2 * left + 1, 2 * right),
      (2 * opposite, 2 * opposite + 1),
  )

  def load_x(b):
    rows = pl.ds(b * SQ, SQ)
    load(("x", b), x_hbm.at[rows], x_f32.at[rows])

  def load_own_kv(b):
    load(("kv", 0, b), kt_hbm.at[b, pl.ds(2 * my, 2)], kt_f32.at[0, b])
    load(("kv", 0, b), vt_hbm.at[b, pl.ds(2 * my, 2)], vt_f32.at[0, b])

  load_x(0)
  load_own_kv(0)

  def remote(buf, stage, rows, send, recv, k, e):
    src = buf.at[1, e, rows] if stage == 3 else buf.at[0, e if stage == 1 else 1 - e, rows]
    to = neighbour[e] if isinstance(e, int) else jnp.where(e == 0, right, left)
    return pltpu.make_async_remote_copy(
        src, buf.at[stage, e, rows], send.at[e, k], recv.at[e, k], device_id=(to,), device_id_type=MESH)

  def hop(*args):
    return [remote(*args, e) for e in range(2)]

  whole = pl.ds(HEADER, PACKET_ROWS - HEADER)
  wq_rows = [pl.ds(BODY + 8 * carrier_at[c], 8 * (carrier_at[c + 1] - carrier_at[c])) for c in range(n_chunks)]
  wq_rows.append(pl.ds(HEADER, BODY - HEADER))
  wq1 = [hop(wq_pkt, 1, rows, wq_send, wq_recv, k) for k, rows in enumerate(wq_rows)]
  wq2 = hop(wq_pkt, 2, whole, wq_send, wq_recv, n_chunks + 1)
  wq3 = hop(wq_pkt, 3, whole, wq_send, wq_recv, n_chunks + 2)
  wo1 = hop(wo_pkt, 1, whole, wo_send, wo_recv, 0)
  wo2 = hop(wo_pkt, 2, whole, wo_send, wo_recv, 1)
  tail_at = [HEADER] + [BODY + 24 * g for g in WO_TAIL[1:]]
  wo3 = [hop(wo_pkt, 3, pl.ds(a, b - a), wo_send, wo_recv, 2 + k)
         for k, (a, b) in enumerate(zip(tail_at, tail_at[1:]))]

  def send_first(k, e):
    remote(wq_pkt, 1, wq_rows[k], wq_send, wq_recv, k, e).start()

  def send_second(e):
    remote(wq_pkt, 2, whole, wq_send, wq_recv, n_chunks + 1, e).start()

  at_once = (my != 0, my == 2)
  pieces = []
  seen = None
  for i, e in enumerate(pair_order):
    rel = {}
    for c in range(n_chunks):
      loaded(("wq", i, c))
      if c == 0:
        lowest = _lowest_exponent(wq_f32[i, pl.ds(0, 16 * WQ_CHUNKS[0]), :], 4.0)
      for w in range(word_at[c], word_at[c + 1]):
        rel[w] = _to_words(wq_f32[i, pl.ds(16 * w, 16), :]) - _offset(lowest)
        seen = rel[w] if seen is None else seen | rel[w]
      _write_carriers(wq_pkt.at[0, e], rel, range(carrier_at[c], carrier_at[c + 1]))
      if i == 0 and c == 0:
        @pl.when(odd)
        def _():
          pl.semaphore_wait(barrier, 1)

        @pl.when(my == 2)
        def _():
          pl.semaphore_wait(barrier, 2)
          for n in neighbour:
            pl.semaphore_signal(ready_sem, 1, device_id=(n,), device_id_type=MESH)

      @pl.when(at_once[i])
      def _():
        send_first(c, e)

    pieces.append((rel, lowest))
  unlisted = None
  for e, (rel, lowest) in zip(pair_order, pieces):
    places, rest = _list_clear_bits(rel)
    unlisted = rest if unlisted is None else unlisted | rest
    _write_header(wq_pkt.at[0, e], places, lowest)
  for i, e in enumerate(pair_order):
    @pl.when(at_once[i])
    def _():
      send_first(n_chunks, e)
      send_second(e)

  load("wo", wo_hbm, wo_f32)
  load_x(1)
  load_own_kv(1)
  for s in range(1, 4):
    for e in range(2):
      load(("kv", s), kt_hbm.at[:, pairs[s][e]], kt_f32.at[s, :, e])
      load(("kv", s), vt_hbm.at[:, pairs[s][e]], vt_f32.at[s, :, e])

  @pl.when(odd)
  def _():
    pl.semaphore_wait(ready_sem, 1)

  @pl.when(my == 0)
  def _():
    pl.semaphore_wait(barrier, 2)

  for i, e in enumerate(pair_order):
    @pl.when(jnp.logical_not(at_once[i]))
    def _():
      for k in range(n_chunks + 1):
        send_first(k, e)
      send_second(e)

  def pack_wo(seen, unlisted):
    headers = []
    for e in range(2):
      tiles = [wo_f32[pl.ds(PAIR * e, PAIR), pl.ds(128 * j, 128)] for j in range(4)]
      low = _lowest_exponent(jnp.concatenate(tiles, axis=0), 1.0 + 2.0**-8)
      rel = {}
      for w in range(WORDS):
        j, i = divmod(w, 8)
        rel[w] = _to_words(tiles[j][16 * i:16 * (i + 1)]) - _offset(low)
        seen = seen | rel[w]
      _write_carriers(wo_pkt.at[0, e], rel, range(3 * WORDS // 4))
      places, rest = _list_clear_bits(rel)
      unlisted = unlisted | rest
      headers.append((places, low))
    lost = (seen & _u32(_bits(12, 3))) | unlisted
    failed = jnp.max((lost != 0).astype(I32), axis=0, keepdims=True).astype(U32)
    for e, (places, low) in enumerate(headers):
      _write_header(wo_pkt.at[0, e], places, low | (failed << _u32(8)))

  low_half = lax.broadcasted_iota(I32, (1, PAIR), 1) < DH
  keep = []
  for j in (1, 2):
    ok = [_allowed(4 * my + j, kb).astype(I32) for kb in range(4)]
    keep.append(jnp.concatenate(
        [jnp.where(low_half, ok[2 * t], ok[2 * t + 1]) != 0 for t in range(2)], axis=1))
  second_block = 3 - lax.rem(4 * my, 3)

  def two_blocks(t):
    other = jnp.where(second_block == 1, t[:, :2 * BLK], t[:, 2 * BLK:])
    other = pltpu.roll(other, jnp.where(second_block == 2, BLK, 0), 1)
    return jnp.where(low_half, t[:, :2 * BLK], other)

  def per_head(q):
    return jnp.concatenate([jnp.where(low_half, q, 0.0), jnp.where(low_half, 0.0, q)], axis=0).astype(BF16)

  def project_q(s, wq, rows):
    q_buf[s, rows, :] = jnp.dot(x_f32[rows, :].astype(BF16), wq, preferred_element_type=F32)

  def query_rows(b):
    return pl.ds(b * SQ, BLK), pl.ds(b * SQ + BLK, 2 * BLK), pl.ds(b * SQ + 3 * BLK, BLK)

  def numerators(s, b):
    first, middle, last = query_rows(b)
    cols = [pl.ds(PAIR * e, PAIR) for e in range(2)]
    k = [kt_f32[s, b, e] * SCORE_SCALE for e in range(2)]
    inner = [jnp.dot(per_head(q_buf[s, middle, cols[e]]), k[e].astype(BF16), preferred_element_type=F32)
             for e in range(2)]
    outer = [jnp.dot(per_head(jnp.concatenate([q_buf[s, first, cols[e]], q_buf[s, last, cols[e]]], axis=0)),
                     two_blocks(k[e]).astype(BF16), preferred_element_type=F32)
             for e in range(2)]
    inner = [jnp.concatenate([jnp.where(keep[i % 2], t[BLK * i:BLK * (i + 1)], MASKED) for i in range(4)], axis=0)
             for t in inner]
    return [[jnp.exp2(t - jnp.max(t, axis=1, keepdims=True)) for t in scores] for scores in (inner, outer)]

  def context(s, b, parts):
    first, middle, last = query_rows(b)
    for is_outer, p in enumerate(parts):
      for h in range(2):
        r = []
        for e in range(2):
          v = vt_f32[s, b, e, pl.ds(DH * h, DH), :]
          v = two_blocks(v) if is_outer else v
          one = jnp.ones_like(v)
          v = jnp.concatenate([one, v] if e else [v, one], axis=0)
          r.append(lax.dot_general(p[e][2 * BLK * h:2 * BLK * (h + 1)].astype(BF16), v.astype(BF16),
                                   (((1,), (1,)), ((), ())), preferred_element_type=F32))
        total = jnp.where(low_half, r[1], r[0])
        scale = pl.reciprocal(total, approx=True)
        scale = scale * (2.0 - total * scale)
        ctx = jnp.where(low_half, r[0], r[1]) * pltpu.roll(scale, DH, 1)
        cols = pl.ds(PAIR * h, PAIR)
        if is_outer:
          ctx_buf[s, first, cols] = ctx[:BLK]
          ctx_buf[s, last, cols] = ctx[BLK:]
        else:
          ctx_buf[s, middle, cols] = ctx

  def attend(s, batches):
    for b, parts in zip(batches, [numerators(s, b) for b in batches]):
      context(s, b, parts)

  def wq_stage(s):
    return jnp.concatenate(
        [_read_words(wq_pkt.at[s, e], _read_header(wq_pkt.at[s, e]), range(WORDS)) for e in range(2)], axis=1)

  flags = []

  def wo_headers(s):
    headers = [_read_header(wo_pkt.at[s, e]) for e in range(2)]
    flags.extend(header[2] for header in headers)
    return headers

  def wo_rows(s, headers, groups):
    return jnp.concatenate(
        [_read_words(wo_pkt.at[s, e], headers[e], range(4 * g, 4 * g + 4)) for g in groups for e in range(2)], axis=0)

  def project_out(s):
    headers = wo_headers(s)
    wo = jnp.concatenate([wo_rows(s, headers, (2 * j, 2 * j + 1)) for j in range(4)], axis=1)
    return jnp.dot(ctx_buf[s].astype(BF16), wo, preferred_element_type=F32)

  def start(copies):
    for copy in copies:
      copy.start()

  def received(copies):
    for copy in copies:
      copy.wait_recv()

  def sent(copies):
    for copy in copies:
      copy.wait_send()

  everything = pl.ds(0, ROWS)

  loaded(("x", 0))
  project_q(0, wq_stage(0), pl.ds(0, SQ))
  loaded(("kv", 0, 0))
  attend(0, [0])
  loaded("wo")
  pack_wo(seen, unlisted)
  start(wo1)
  loaded(("x", 1))
  project_q(0, wq_stage(0), pl.ds(SQ, SQ))
  loaded(("kv", 0, 1))
  attend(0, [1])

  for copies in wq1:
    received(copies)
  start(wq3)
  start(wo2)
  project_q(1, wq_stage(1), everything)
  loaded(("kv", 1))
  attend(1, [0, 1])

  loaded(("kv", 2))
  received(wq2)
  project_q(2, wq_stage(2), everything)
  attend(2, [0, 1])

  received(wo1)
  for copies in wo3:
    start(copies)
  acc_buf[...] = project_out(0) + project_out(1)

  loaded(("kv", 3))
  received(wq3)
  project_q(3, wq_stage(3), everything)
  attend(3, [0, 1])

  received(wo2)
  acc_buf[...] += project_out(2)

  for copies in (*wq1, wq2, wq3, wo1, wo2):
    sent(copies)
  for copies, g0, g1 in zip(wo3, WO_TAIL, WO_TAIL[1:]):
    sent(copies)
    received(copies)
    if g0 == 0:
      headers = wo_headers(3)
      failed = flags[0]
      for flag in flags[1:]:
        failed = failed | flag
      failed = jnp.max(failed.astype(I32)) > 0
    if g1 - g0 > 1:
      wo = jnp.concatenate([wo_rows(3, headers, (g, g + 1)) for g in range(g0, g1, 2)], axis=1)
      heads = pl.ds(0, 2 * PAIR)
    else:
      wo = wo_rows(3, headers, (g0,))
      heads = pl.ds(PAIR * (g0 % 2), PAIR)
    cols = pl.ds(128 * (g0 // 2), wo.shape[1])
    parts = 4 // (g1 - g0)
    for i in range(parts):
      rows = pl.ds(i * ROWS // parts, ROWS // parts)
      total = acc_buf[rows, cols] + jnp.dot(ctx_buf[3, rows, heads].astype(BF16), wo, preferred_element_type=F32)
      if g1 % 2:
        acc_buf[rows, cols] = total
      else:
        out_ref[rows, cols] = total.astype(out_ref.dtype)

  @pl.when(failed)
  def _():
    for e in range(2):
      wq_raw[0, pair_order[e]] = _to_words(wq_f32[e])
      wo_raw[0, e] = _to_words(wo_f32[pl.ds(PAIR * e, PAIR), :])
    hops = [hop(wq_raw, s, pl.ds(0, D // 2), raw_send, raw_recv, 2 * s - 2)
            + hop(wo_raw, s, pl.ds(0, PAIR // 2), raw_send, raw_recv, 2 * s - 1) for s in (1, 2, 3)]
    start(hops[0] + hops[1])
    received(hops[0])
    start(hops[2])
    received(hops[1] + hops[2])
    sent(hops[0] + hops[1] + hops[2])
    acc_buf[...] = jnp.zeros_like(acc_buf)

    @pl.loop(0, 4)
    def _(s):
      project_q(s, jnp.concatenate([_from_words(wq_raw[s, e]) for e in range(2)], axis=1), everything)

      @pl.loop(0, B)
      def _(b):
        attend(s, [b])

      wo = jnp.concatenate(
          [_from_words(wo_raw[s, e, pl.ds(DH // 2 * h, DH // 2), :]) for h in range(2) for e in range(2)], axis=0)
      acc_buf[...] += jnp.dot(ctx_buf[s].astype(BF16), wo, preferred_element_type=F32)

    out_ref[...] = acc_buf[...].astype(out_ref.dtype)


def pallas_dist_sparse_attn_blocksparse_qseq_b2_sq256_skv256_hq4_dh64_kernel(
    x: jax.Array,
    Wq: jax.Array,
    K_ext: jax.Array,
    V_ext: jax.Array,
    Wo: jax.Array,
):
  kt = jnp.transpose(K_ext, (0, 2, 3, 1)).reshape(B, 2 * N_DEV, PAIR, SKV)
  vt = jnp.transpose(V_ext, (0, 2, 3, 1)).reshape(B, 2 * N_DEV, PAIR, SKV)
  n_chunks, n_tail = len(WQ_CHUNKS), len(WO_TAIL) - 1
  out = pl.pallas_call(
      _kernel,
      out_shape=pltpu.VMEM((ROWS, D), BF16),
      in_specs=[pl.BlockSpec(memory_space=pl.ANY)] * 5,
      out_specs=pl.BlockSpec(memory_space=pltpu.VMEM),
      scratch_shapes=[
          pltpu.VMEM((ROWS, D), F32),
          pltpu.VMEM((2, D, PAIR), F32),
          pltpu.VMEM((2 * PAIR, D), F32),
          pltpu.VMEM((4, B, 2, PAIR, SKV), F32),
          pltpu.VMEM((4, B, 2, PAIR, SKV), F32),
          pltpu.VMEM((4, ROWS, 2 * PAIR), F32),
          pltpu.VMEM((4, ROWS, 2 * PAIR), F32),
          pltpu.VMEM((ROWS, D), F32),
          pltpu.VMEM((4, 2, PACKET_ROWS, 128), U32),
          pltpu.VMEM((4, 2, PACKET_ROWS, 128), U32),
          pltpu.VMEM((4, 2, D // 2, PAIR), U32),
          pltpu.VMEM((4, 2, PAIR // 2, D), U32),
          pltpu.SemaphoreType.DMA((2 * n_chunks + 19,)),
          pltpu.SemaphoreType.DMA((2, n_chunks + 3)),
          pltpu.SemaphoreType.DMA((2, n_chunks + 3)),
          pltpu.SemaphoreType.DMA((2, n_tail + 2)),
          pltpu.SemaphoreType.DMA((2, n_tail + 2)),
          pltpu.SemaphoreType.DMA((2, 6)),
          pltpu.SemaphoreType.DMA((2, 6)),
          pltpu.SemaphoreType.REGULAR,
      ],
      compiler_params=pltpu.CompilerParams(
          collective_id=0,
          vmem_limit_bytes=48 * 1024 * 1024,
          disable_semaphore_checks=True,
      ),
  )(x.reshape(ROWS, D), Wq, kt, vt, Wo)
  return out.reshape(B, SQ, D)
```
